```python
import numpy as np

kernel_name = "dist_argmax_global_i_m4096_n1024"

def setup_inputs():
    return {"x": np.random.randn(16384, 1024).astype(np.float32)}

def reference(x: np.ndarray) -> np.ndarray:
    idx = np.argmax(x, axis=0).astype(np.float32)
    val = np.max(x, axis=0)
    return np.stack([val, idx], axis=0)
```

```python
import functools

import jax
import jax.numpy as jnp
from jax import lax
from jax.experimental import pallas as pl
from jax.experimental.pallas import tpu as pltpu

N_DEV = 4
SUB = 8
LANES = 128
NO_ROW = 2**30
PEER_ROWS = 208
N_IN_SEMS = 3
N_CHAINS = 4
SEND_ORDER = (2, 1, 3)


def _step(x, cur, best, grp):
    keep = jnp.logical_or(x <= best, best != best)
    return jnp.where(keep, best, x), jnp.where(keep, grp, cur)


def _is_hit(v, vmax):
    return jnp.logical_or(v == vmax, v != v)


def _merge(states):
    vmax = functools.reduce(jnp.maximum, [v for v, _ in states])
    none = jnp.asarray(NO_ROW, states[0][1].dtype)
    idx = functools.reduce(jnp.minimum, [jnp.where(_is_hit(v, vmax), i, none) for v, i in states])
    return vmax, idx


def _schedule(m, n):
    ca = n - LANES
    r0 = 3 * m // 4
    tail = m - r0
    full = [m // 2 - 2 * PEER_ROWS, m // 4]
    a_rows = [3 * tail // 4, tail // 4]
    b_rows = [3 * tail // 4, 7 * tail // 32, tail // 32]
    pieces, r = [], 2 * PEER_ROWS
    for rows in full:
        pieces.append((r, rows, 0, n))
        r += rows
    assert r == r0
    for rows in a_rows:
        pieces.append((r, rows, 0, ca))
        r += rows
    assert r == m
    r = r0
    for rows in b_rows:
        pieces.append((r, rows, ca, n - ca))
        r += rows
    assert r == m
    return pieces, len(full), len(a_rows), ca


def pallas_dist_argmax_global_i_m4096_n1024_kernel(
    x: jax.Array,
):
    m, n = x.shape
    pieces, n_full, n_a, ca = _schedule(m, n)
    cb = n - ca
    n_pieces = len(pieces)
    groups_per_dev = m // SUB

    def kernel_body(
        x_hbm, o_ref, buf, peer, send_a, send_b, recv_a, recv_b, in_sems, send_sem, recv_sems
    ):
        me = lax.axis_index("i")
        my_grp0 = me * groups_per_dev

        def fetch(i):
            r0, rows, c0, cols = pieces[i]
            return pltpu.make_async_copy(
                x_hbm.at[pl.ds(r0, rows), pl.ds(c0, cols)],
                buf.at[pl.ds(r0, rows), pl.ds(c0, cols)],
                in_sems.at[i % N_IN_SEMS],
            )

        def remote(src, dst, recv_sem, dist):
            return pltpu.make_async_remote_copy(
                src_ref=src,
                dst_ref=dst,
                send_sem=send_sem.at[0],
                recv_sem=recv_sem,
                device_id=((me + dist) % N_DEV,),
                device_id_type=pl.DeviceIdType.MESH,
            )

        for i in range(min(N_IN_SEMS, n_pieces)):
            fetch(i).start()

        barrier = pltpu.get_barrier_semaphore()
        for dist in range(1, N_DEV):
            pl.semaphore_signal(
                barrier,
                inc=1,
                device_id=((me + dist) % N_DEV,),
                device_id_type=pl.DeviceIdType.MESH,
            )
        pl.semaphore_wait(barrier, N_DEV - 1)

        sends = []
        for k, dist in enumerate((1, N_DEV - 1)):
            push = remote(x_hbm.at[pl.ds(k * PEER_ROWS, PEER_ROWS)], peer.at[k], recv_sems.at[2], dist)
            push.start()
            sends.append(push)

        def scan(load, grp0, g0, n_groups, state):
            unroll = 2 if n_groups % 2 == 0 else 1

            def body(t, carry):
                for u in range(unroll):
                    g = g0 + t * unroll + u
                    carry = _step(load(g), jnp.full(carry[1].shape, grp0 + g, jnp.int32), *carry)
                return carry

            if n_groups == unroll:
                return body(0, state)
            return lax.fori_loop(0, n_groups // unroll, body, state)

        def scan_own(i, state):
            r0, rows, c0, cols = pieces[i]

            def load(g):
                return buf[pl.ds(pl.multiple_of(g * SUB, SUB), SUB), pl.ds(c0, cols)]

            return scan(load, my_grp0, r0 // SUB, rows // SUB, state)

        def scan_own_chains(i, chains):
            r0, rows, c0, cols = pieces[i]
            chains = list(chains)
            for t in range(rows // SUB):
                xg = buf[pl.ds(r0 + t * SUB, SUB), pl.ds(c0, cols)]
                cur = jnp.full((SUB, cols), my_grp0 + r0 // SUB + t, jnp.int32)
                chains[t % len(chains)] = _step(xg, cur, *chains[t % len(chains)])
            return chains

        def empty(cols, grp):
            return jnp.full((SUB, cols), -jnp.inf, jnp.float32), jnp.zeros((SUB, cols), jnp.int32) + grp

        def finish_local(state, dst):
            best, grp = state
            row = grp * SUB + lax.broadcasted_iota(jnp.int32, best.shape, 0)
            vmax = jnp.max(best, axis=0, keepdims=True)
            idx = jnp.min(jnp.where(_is_hit(best, vmax), row, NO_ROW), axis=0, keepdims=True)
            idx = idx.astype(jnp.float32)
            dst[0:1, :] = vmax
            dst[1:2, :] = idx
            return vmax, idx

        def send_partial(src, dst, recv_sem):
            copies = [remote(src, dst.at[dist - 1], recv_sem, dist) for dist in SEND_ORDER]
            for c in copies:
                c.start()
            return copies

        def finish_global(mine, recv, c0, cols):
            parts = [mine] + [(recv[s, 0:1, :], recv[s, 1:2, :]) for s in range(N_DEV - 1)]
            vmax, idx = _merge(parts)
            o_ref[0:1, pl.ds(c0, cols)] = vmax
            o_ref[1:2, pl.ds(c0, cols)] = idx

        state = state_a = chains_b = mine_a = None
        for i in range(n_pieces):
            fetch(i).wait()
            if i + N_IN_SEMS < n_pieces:
                fetch(i + N_IN_SEMS).start()
            if i < n_full:
                if i == 0:
                    state = empty(n, my_grp0 + pieces[0][0] // SUB)
                state = scan_own(i, state)
                if i == n_full - 1:
                    state_a = (state[0][:, :ca], state[1][:, :ca])
                    chains_b = [(state[0][:, ca:], state[1][:, ca:])]
                    chains_b += [empty(cb, NO_ROW) for _ in range(N_CHAINS - 1)]
            elif i < n_full + n_a:
                state_a = scan_own(i, state_a)
            else:
                chains_b = scan_own_chains(i, chains_b)
                if i == n_pieces - 2:
                    chains_b = [_merge(chains_b)]

            if i == n_full:
                pltpu.make_async_copy(peer, peer, recv_sems.at[2]).wait()
                theirs = []
                for k, dist in enumerate((N_DEV - 1, 1)):
                    grp0 = ((me + dist) % N_DEV) * groups_per_dev + k * (PEER_ROWS // SUB)

                    def load(g, k=k):
                        return peer[k, pl.ds(pl.multiple_of(g * SUB, SUB), SUB), :]

                    theirs.append(scan(load, grp0, 0, PEER_ROWS // SUB, empty(n, grp0)))
                vmax, grp = _merge(theirs)
                state_a = _merge([state_a, (vmax[:, :ca], grp[:, :ca])])
                chains_b[0] = _merge([chains_b[0], (vmax[:, ca:], grp[:, ca:])])
            if i == n_full + n_a - 1:
                mine_a = finish_local(state_a, send_a)
                sends += send_partial(send_a, recv_a, recv_sems.at[0])

        mine_b = finish_local(chains_b[0], send_b)
        sends += send_partial(send_b, recv_b, recv_sems.at[1])

        pltpu.make_async_copy(recv_a, recv_a, recv_sems.at[0]).wait()
        finish_global(mine_a, recv_a, 0, ca)
        pltpu.make_async_copy(recv_b, recv_b, recv_sems.at[1]).wait()
        finish_global(mine_b, recv_b, ca, cb)
        for c in sends:
            c.wait_send()

    return pl.pallas_call(
        kernel_body,
        out_shape=jax.ShapeDtypeStruct((2, n), jnp.float32),
        in_specs=[pl.BlockSpec(memory_space=pl.ANY)],
        out_specs=pl.BlockSpec(memory_space=pltpu.VMEM),
        scratch_shapes=[
            pltpu.VMEM((m, n), jnp.float32),
            pltpu.VMEM((2, PEER_ROWS, n), jnp.float32),
            pltpu.VMEM((2, ca), jnp.float32),
            pltpu.VMEM((2, cb), jnp.float32),
            pltpu.VMEM((N_DEV - 1, 2, ca), jnp.float32),
            pltpu.VMEM((N_DEV - 1, 2, cb), jnp.float32),
            pltpu.SemaphoreType.DMA((N_IN_SEMS,)),
            pltpu.SemaphoreType.DMA((1,)),
            pltpu.SemaphoreType.DMA((3,)),
        ],
        compiler_params=pltpu.CompilerParams(
            vmem_limit_bytes=64 * 1024 * 1024,
            collective_id=0,
        ),
    )(x)
```

```python
import jax
import jax.numpy as jnp
from jax import lax
from jax.experimental import pallas as pl
from jax.experimental.pallas import tpu as pltpu

N_DEV = 4
SUB = 8
COLS_B = 128
NO_ROW = 2**30
PEER_ROWS = 208
N_IN_SEMS = 3
N_CHAINS = 4
SEND_ORDER = (2, 1, 3)


def _tree(fn, xs):
    while len(xs) > 1:
        xs = [fn(*xs[i : i + 2]) if i + 1 < len(xs) else xs[i] for i in range(0, len(xs), 2)]
    return xs[0]


def _step(x, cur, best, grp):
    keep = jnp.logical_or(x <= best, best != best)
    return jnp.where(keep, best, x), jnp.where(keep, grp, cur)


def _candidates(v, idx, vmax):
    return jnp.where(jnp.logical_or(v == vmax, v != v), idx, NO_ROW)


def _merge(states):
    vmax = _tree(jnp.maximum, [v for v, _ in states])
    return vmax, _tree(jnp.minimum, [_candidates(v, i, vmax) for v, i in states])


def _schedule(m, n):
    split = 3 * m // 4
    tail = m - split
    cols_a = n - COLS_B
    plan = (
        (2 * PEER_ROWS, (m // 2 - 2 * PEER_ROWS, m // 4), 0, n, split),
        (split, (3 * tail // 4, tail // 4), 0, cols_a, m),
        (split, (3 * tail // 4, 7 * tail // 32, tail // 32), cols_a, COLS_B, m),
    )
    pieces = []
    for r, sizes, c0, cols, end in plan:
        for rows in sizes:
            assert rows % SUB == 0
            pieces.append((r, rows, c0, cols))
            r += rows
        assert r == end
    return pieces, len(plan[0][1]), len(plan[1][1])


def pallas_dist_argmax_global_i_m4096_n1024_kernel(
    x: jax.Array,
):
    m, n = x.shape
    pieces, n_full, n_a = _schedule(m, n)
    n_pieces = len(pieces)
    cols_a = n - COLS_B
    groups_per_dev = m // SUB

    def kernel_body(x_hbm, o_ref, buf, peer, send_a, send_b, recv_a, recv_b):
        me = lax.axis_index("i")
        my_grp0 = me * groups_per_dev

        def ring(dist):
            return jnp.bitwise_and(me + dist, N_DEV - 1)

        def remote(src, dst, send_sem, recv_sem, dist):
            return pltpu.make_async_remote_copy(
                src_ref=src,
                dst_ref=dst,
                send_sem=send_sem,
                recv_sem=recv_sem,
                device_id=(ring(dist),),
                device_id_type=pl.DeviceIdType.MESH,
            )

        def empty(cols, grp):
            return (
                jnp.full((SUB, cols), -jnp.inf, jnp.float32),
                jnp.zeros((SUB, cols), jnp.int32) + grp,
            )

        def scan(load, grp0, g0, n_groups, state):
            unroll = 2 if n_groups % 2 == 0 else 1

            def body(t, carry):
                for u in range(unroll):
                    g = g0 + t * unroll + u
                    cur = jnp.full(carry[1].shape, grp0 + g, jnp.int32)
                    carry = _step(load(g), cur, *carry)
                return carry

            return lax.fori_loop(0, n_groups // unroll, body, state)

        def scan_own(i, state):
            r0, rows, c0, cols = pieces[i]

            def load(g):
                return buf[pl.ds(pl.multiple_of(g * SUB, SUB), SUB), pl.ds(c0, cols)]

            return scan(load, my_grp0, r0 // SUB, rows // SUB, state)

        def scan_own_chains(i, chains):
            r0, rows, c0, cols = pieces[i]
            chains = list(chains)
            for t in range(rows // SUB):
                xg = buf[pl.ds(r0 + t * SUB, SUB), pl.ds(c0, cols)]
                cur = jnp.full((SUB, cols), my_grp0 + r0 // SUB + t, jnp.int32)
                chains[t % len(chains)] = _step(xg, cur, *chains[t % len(chains)])
            return chains

        def scan_peers():
            theirs = []
            for k, dist in enumerate((N_DEV - 1, 1)):
                grp0 = ring(dist) * groups_per_dev + k * (PEER_ROWS // SUB)

                def load(g, k=k):
                    return peer[k, pl.ds(pl.multiple_of(g * SUB, SUB), SUB), :]

                theirs.append(scan(load, grp0, 0, PEER_ROWS // SUB, empty(n, grp0)))
            return _merge(theirs)

        def finish_local(states, dst):
            sub = lax.broadcasted_iota(jnp.int32, dst_shape(dst), 0)
            vmax = jnp.max(_tree(jnp.maximum, [v for v, _ in states]), axis=0, keepdims=True)
            rows = [
                _candidates(v, (grp * SUB + sub).astype(jnp.float32), vmax) for v, grp in states
            ]
            idx = jnp.min(_tree(jnp.minimum, rows), axis=0, keepdims=True)
            dst[0:1, :] = vmax
            dst[1:2, :] = idx
            return vmax, idx

        def dst_shape(dst):
            return (SUB, dst.shape[1])

        def send_partial(src, dst, send_sem, recv_sem):
            copies = [remote(src, dst.at[d - 1], send_sem, recv_sem, d) for d in SEND_ORDER]
            for c in copies:
                c.start()
            return copies

        def finish_global(mine, recv, c0, cols):
            parts = [mine] + [(recv[s, 0:1, :], recv[s, 1:2, :]) for s in range(N_DEV - 1)]
            vmax, idx = _merge(parts)
            o_ref[0:1, pl.ds(c0, cols)] = vmax
            o_ref[1:2, pl.ds(c0, cols)] = idx

        def run(in_sems, send_sem, peer_sem, recv_a_sem, recv_b_sem):
            def fetch(i):
                r0, rows, c0, cols = pieces[i]
                return pltpu.make_async_copy(
                    x_hbm.at[pl.ds(r0, rows), pl.ds(c0, cols)],
                    buf.at[pl.ds(r0, rows), pl.ds(c0, cols)],
                    in_sems.at[i % N_IN_SEMS],
                )

            for i in range(N_IN_SEMS):
                fetch(i).start()

            barrier = pltpu.get_barrier_semaphore()
            for dist in range(1, N_DEV):
                pl.semaphore_signal(
                    barrier, inc=1, device_id=(ring(dist),), device_id_type=pl.DeviceIdType.MESH
                )
            pl.semaphore_wait(barrier, N_DEV - 1)

            sends = []
            for k, dist in enumerate((1, N_DEV - 1)):
                src = x_hbm.at[pl.ds(k * PEER_ROWS, PEER_ROWS)]
                sends.append(remote(src, peer.at[k], send_sem, peer_sem, dist))
                sends[-1].start()

            state = state_a = chains_b = peer_a = peer_b = mine_a = None
            for i in range(n_pieces):
                fetch(i).wait()
                if i + N_IN_SEMS < n_pieces:
                    fetch(i + N_IN_SEMS).start()
                if i < n_full:
                    if i == 0:
                        state = empty(n, my_grp0 + pieces[0][0] // SUB)
                    state = scan_own(i, state)
                    if i == n_full - 1:
                        state_a = (state[0][:, :cols_a], state[1][:, :cols_a])
                        chains_b = [(state[0][:, cols_a:], state[1][:, cols_a:])]
                        chains_b += [empty(COLS_B, NO_ROW) for _ in range(N_CHAINS - 1)]
                elif i < n_full + n_a:
                    state_a = scan_own(i, state_a)
                else:
                    chains_b = scan_own_chains(i, chains_b)
                    if i == n_pieces - 2:
                        chains_b = [_merge(chains_b)]

                if i == n_full:
                    pltpu.make_async_copy(peer, peer, peer_sem).wait()
                    vmax, grp = scan_peers()
                    peer_a = (vmax[:, :cols_a], grp[:, :cols_a])
                    peer_b = (vmax[:, cols_a:], grp[:, cols_a:])
                if i == n_full + n_a - 1:
                    mine_a = finish_local([state_a, peer_a], send_a)
                    sends += send_partial(send_a, recv_a, send_sem, recv_a_sem)

            mine_b = finish_local([chains_b[0], peer_b], send_b)
            last_sends = send_partial(send_b, recv_b, send_sem, recv_b_sem)

            pltpu.make_async_copy(recv_a, recv_a, recv_a_sem).wait()
            finish_global(mine_a, recv_a, 0, cols_a)
            pltpu.make_async_copy(recv_b, recv_b, recv_b_sem).wait()
            finish_global(mine_b, recv_b, cols_a, COLS_B)
            for c in sends + last_sends:
                c.wait_send()

        pl.run_scoped(
            run,
            pltpu.SemaphoreType.DMA((N_IN_SEMS,)),
            pltpu.SemaphoreType.DMA,
            pltpu.SemaphoreType.DMA,
            pltpu.SemaphoreType.DMA,
            pltpu.SemaphoreType.DMA,
        )

    return pl.pallas_call(
        kernel_body,
        out_shape=jax.ShapeDtypeStruct((2, n), jnp.float32),
        in_specs=[pl.BlockSpec(memory_space=pl.ANY)],
        out_specs=pl.BlockSpec(memory_space=pltpu.VMEM),
        scratch_shapes=[
            pltpu.VMEM((m, n), jnp.float32),
            pltpu.VMEM((2, PEER_ROWS, n), jnp.float32),
            pltpu.VMEM((2, cols_a), jnp.float32),
            pltpu.VMEM((2, COLS_B), jnp.float32),
            pltpu.VMEM((N_DEV - 1, 2, cols_a), jnp.float32),
            pltpu.VMEM((N_DEV - 1, 2, COLS_B), jnp.float32),
        ],
        compiler_params=pltpu.CompilerParams(
            vmem_limit_bytes=64 * 1024 * 1024,
            collective_id=0,
        ),
    )(x)
```

```python
import jax
import jax.numpy as jnp
from jax import lax
from jax.experimental import pallas as pl
from jax.experimental.pallas import tpu as pltpu

N_DEV = 4
SUB = 8
COLS_B = 128
NO_ROW = 2**30
PEER_ROWS = 192
N_IN_SEMS = 3
N_CHAINS = 4
SEND_ORDER = (2, 1, 3)


def _tree(fn, xs):
    while len(xs) > 1:
        xs = [fn(*xs[i : i + 2]) if i + 1 < len(xs) else xs[i] for i in range(0, len(xs), 2)]
    return xs[0]


def _step(x, cur, best, grp):
    keep = jnp.logical_or(x <= best, best != best)
    return jnp.where(keep, best, x), jnp.where(keep, grp, cur)


def _candidates(v, idx, vmax):
    return jnp.where(jnp.logical_or(v == vmax, v != v), idx, NO_ROW)


def _merge(states):
    vmax = _tree(jnp.maximum, [v for v, _ in states])
    return vmax, _tree(jnp.minimum, [_candidates(v, i, vmax) for v, i in states])


def _schedule(m, n):
    split = 3 * m // 4
    tail = m - split
    cols_a = n - COLS_B
    plan = (
        (2 * PEER_ROWS, (m // 2 - 2 * PEER_ROWS, m // 4), 0, n, split),
        (split, (3 * tail // 4, tail // 4), 0, cols_a, m),
        (split, (3 * tail // 4, 7 * tail // 32, tail // 32), cols_a, COLS_B, m),
    )
    pieces = []
    for r, sizes, c0, cols, end in plan:
        for rows in sizes:
            assert rows % SUB == 0
            pieces.append((r, rows, c0, cols))
            r += rows
        assert r == end
    return pieces, len(plan[0][1]), len(plan[1][1])


def pallas_dist_argmax_global_i_m4096_n1024_kernel(
    x: jax.Array,
):
    m, n = x.shape
    pieces, n_full, n_a = _schedule(m, n)
    n_pieces = len(pieces)
    cols_a = n - COLS_B
    groups_per_dev = m // SUB

    def kernel_body(x_hbm, o_ref, buf, peer, send_a, send_b, recv_a, recv_b):
        me = lax.axis_index("i")
        my_grp0 = me * groups_per_dev

        def ring(dist):
            return jnp.bitwise_and(me + dist, N_DEV - 1)

        def remote(src, dst, send_sem, recv_sem, dist):
            return pltpu.make_async_remote_copy(
                src_ref=src,
                dst_ref=dst,
                send_sem=send_sem,
                recv_sem=recv_sem,
                device_id=(ring(dist),),
                device_id_type=pl.DeviceIdType.MESH,
            )

        def empty(cols, grp):
            return (
                jnp.full((SUB, cols), -jnp.inf, jnp.float32),
                jnp.zeros((SUB, cols), jnp.int32) + grp,
            )

        def scan(load, grp0, g0, n_groups, state):
            unroll = 2 if n_groups % 2 == 0 else 1

            def body(t, carry):
                for u in range(unroll):
                    g = g0 + t * unroll + u
                    cur = jnp.full(carry[1].shape, grp0 + g, jnp.int32)
                    carry = _step(load(g), cur, *carry)
                return carry

            return lax.fori_loop(0, n_groups // unroll, body, state)

        def scan_own(i, state):
            r0, rows, c0, cols = pieces[i]

            def load(g):
                return buf[pl.ds(pl.multiple_of(g * SUB, SUB), SUB), pl.ds(c0, cols)]

            return scan(load, my_grp0, r0 // SUB, rows // SUB, state)

        def scan_own_chains(i, chains):
            r0, rows, c0, cols = pieces[i]
            chains = list(chains)
            for t in range(rows // SUB):
                xg = buf[pl.ds(r0 + t * SUB, SUB), pl.ds(c0, cols)]
                cur = jnp.full((SUB, cols), my_grp0 + r0 // SUB + t, jnp.int32)
                chains[t % len(chains)] = _step(xg, cur, *chains[t % len(chains)])
            return chains

        def scan_peers():
            theirs = []
            for k, dist in enumerate((N_DEV - 1, 1)):
                grp0 = ring(dist) * groups_per_dev + k * (PEER_ROWS // SUB)

                def load(g, k=k):
                    return peer[k, pl.ds(pl.multiple_of(g * SUB, SUB), SUB), :]

                theirs.append(scan(load, grp0, 0, PEER_ROWS // SUB, empty(n, grp0)))
            return _merge(theirs)

        def finish_local(states, dst):
            sub = lax.broadcasted_iota(jnp.int32, (SUB, dst.shape[1]), 0)
            vmax = jnp.max(_tree(jnp.maximum, [v for v, _ in states]), axis=0, keepdims=True)
            rows = [
                _candidates(v, (grp * SUB + sub).astype(jnp.float32), vmax) for v, grp in states
            ]
            idx = jnp.min(_tree(jnp.minimum, rows), axis=0, keepdims=True)
            dst[0:1, :] = vmax
            dst[1:2, :] = idx
            return vmax, idx

        def send_partial(src, dst, send_sem, recv_sem):
            copies = [remote(src, dst.at[d - 1], send_sem, recv_sem, d) for d in SEND_ORDER]
            for c in copies:
                c.start()
            return copies

        def finish_global(mine, recv, c0, cols):
            parts = [mine] + [(recv[s, 0:1, :], recv[s, 1:2, :]) for s in range(N_DEV - 1)]
            vmax, idx = _merge(parts)
            o_ref[0:1, pl.ds(c0, cols)] = vmax
            o_ref[1:2, pl.ds(c0, cols)] = idx

        def run(in_sems, send_sem, peer_sem, recv_a_sem, recv_b_sem):
            def fetch(i):
                r0, rows, c0, cols = pieces[i]
                return pltpu.make_async_copy(
                    x_hbm.at[pl.ds(r0, rows), pl.ds(c0, cols)],
                    buf.at[pl.ds(r0, rows), pl.ds(c0, cols)],
                    in_sems.at[i % N_IN_SEMS],
                )

            for i in range(N_IN_SEMS):
                fetch(i).start()

            barrier = pltpu.get_barrier_semaphore()
            for dist in range(1, N_DEV):
                pl.semaphore_signal(
                    barrier, inc=1, device_id=(ring(dist),), device_id_type=pl.DeviceIdType.MESH
                )
            pl.semaphore_wait(barrier, N_DEV - 1)

            sends = []
            for k, dist in enumerate((1, N_DEV - 1)):
                src = x_hbm.at[pl.ds(k * PEER_ROWS, PEER_ROWS)]
                sends.append(remote(src, peer.at[k], send_sem, peer_sem, dist))
                sends[-1].start()

            state = state_a = chains_b = peer_a = peer_b = mine_a = None
            for i in range(n_pieces):
                fetch(i).wait()
                if i + N_IN_SEMS < n_pieces:
                    fetch(i + N_IN_SEMS).start()
                if i < n_full:
                    if i == 0:
                        state = empty(n, my_grp0 + pieces[0][0] // SUB)
                    state = scan_own(i, state)
                    if i == n_full - 1:
                        state_a = (state[0][:, :cols_a], state[1][:, :cols_a])
                        chains_b = [(state[0][:, cols_a:], state[1][:, cols_a:])]
                        chains_b += [empty(COLS_B, NO_ROW) for _ in range(N_CHAINS - 1)]
                elif i < n_full + n_a:
                    state_a = scan_own(i, state_a)
                else:
                    chains_b = scan_own_chains(i, chains_b)
                    if i == n_pieces - 2:
                        chains_b = [_merge(chains_b)]

                if i == n_full:
                    pltpu.make_async_copy(peer, peer, peer_sem).wait()
                    vmax, grp = scan_peers()
                    peer_a = (vmax[:, :cols_a], grp[:, :cols_a])
                    peer_b = (vmax[:, cols_a:], grp[:, cols_a:])
                if i == n_full + n_a - 1:
                    mine_a = finish_local([state_a, peer_a], send_a)
                    sends += send_partial(send_a, recv_a, send_sem, recv_a_sem)

            mine_b = finish_local([chains_b[0], peer_b], send_b)
            last_sends = send_partial(send_b, recv_b, send_sem, recv_b_sem)

            pltpu.make_async_copy(recv_a, recv_a, recv_a_sem).wait()
            finish_global(mine_a, recv_a, 0, cols_a)
            pltpu.make_async_copy(recv_b, recv_b, recv_b_sem).wait()
            finish_global(mine_b, recv_b, cols_a, COLS_B)
            for c in sends + last_sends:
                c.wait_send()

        pl.run_scoped(
            run,
            pltpu.SemaphoreType.DMA((N_IN_SEMS,)),
            pltpu.SemaphoreType.DMA,
            pltpu.SemaphoreType.DMA,
            pltpu.SemaphoreType.DMA,
            pltpu.SemaphoreType.DMA,
        )

    return pl.pallas_call(
        kernel_body,
        out_shape=jax.ShapeDtypeStruct((2, n), jnp.float32),
        in_specs=[pl.BlockSpec(memory_space=pl.ANY)],
        out_specs=pl.BlockSpec(memory_space=pltpu.VMEM),
        scratch_shapes=[
            pltpu.VMEM((m, n), jnp.float32),
            pltpu.VMEM((2, PEER_ROWS, n), jnp.float32),
            pltpu.VMEM((2, cols_a), jnp.float32),
            pltpu.VMEM((2, COLS_B), jnp.float32),
            pltpu.VMEM((N_DEV - 1, 2, cols_a), jnp.float32),
            pltpu.VMEM((N_DEV - 1, 2, COLS_B), jnp.float32),
        ],
        compiler_params=pltpu.CompilerParams(
            vmem_limit_bytes=64 * 1024 * 1024,
            collective_id=0,
        ),
    )(x)
```

```python
import jax
import jax.numpy as jnp
from jax import lax
from jax.experimental import pallas as pl
from jax.experimental.pallas import tpu as pltpu

N_DEV = 4
SUB = 8
COLS_B = 128
NO_ROW = 2**30
INF_BITS = 0x7F800000
KEY_NAN = 0x7FFFFFFF
KEY_MIN = -(2**31)
PEER_ROWS = 192
N_IN_SEMS = 3
MAX_UNROLL = 8
N_CHAINS = 4
SEND_ORDER = (2, 1, 3)


def _tree(fn, xs):
    while len(xs) > 1:
        xs = [fn(*xs[i : i + 2]) if i + 1 < len(xs) else xs[i] for i in range(0, len(xs), 2)]
    return xs[0]


def _key(x):
    bits = pltpu.bitcast(x, jnp.int32)
    mag = jnp.bitwise_and(bits, 0x7FFFFFFF)
    sign = jnp.right_shift(bits, 31)
    return jnp.where(mag > INF_BITS, KEY_NAN, jnp.bitwise_xor(mag, sign) - sign)


def _unkey(key):
    bits = jnp.where(key < 0, jnp.bitwise_or(-key, KEY_MIN), key)
    return pltpu.bitcast(bits, jnp.float32)


def _step(x, cur, best, grp):
    key = _key(x)
    take = key > best
    return jnp.where(take, key, best), jnp.where(take, cur, grp)


def _merge(states):
    top = _tree(jnp.maximum, [k for k, _ in states])
    return top, _tree(jnp.minimum, [jnp.where(k == top, i, NO_ROW) for k, i in states])


def _schedule(m, n):
    split = 3 * m // 4
    tail = m - split
    cols_a = n - COLS_B
    plan = (
        (2 * PEER_ROWS, (m // 2 - 2 * PEER_ROWS, m // 4), 0, n, split),
        (split, (tail // 2, 3 * tail // 8, tail // 8), 0, cols_a, m),
        (split, (3 * tail // 4, 7 * tail // 32, tail // 32), cols_a, COLS_B, m),
    )
    pieces = []
    for r, sizes, c0, cols, end in plan:
        for rows in sizes:
            assert rows % SUB == 0
            pieces.append((r, rows, c0, cols))
            r += rows
        assert r == end
    return pieces, len(plan[0][1]), len(plan[1][1])


def pallas_dist_argmax_global_i_m4096_n1024_kernel(
    x: jax.Array,
):
    m, n = x.shape
    pieces, n_full, n_a = _schedule(m, n)
    n_pieces = len(pieces)
    cols_a = n - COLS_B
    groups_per_dev = m // SUB

    def kernel_body(x_hbm, o_ref, buf, peer, send_a, send_b, recv_a, recv_b):
        me = lax.axis_index("i")
        my_grp0 = me * groups_per_dev

        def ring(dist):
            return jnp.bitwise_and(me + dist, N_DEV - 1)

        def remote(src, dst, send_sem, recv_sem, dist):
            return pltpu.make_async_remote_copy(
                src_ref=src,
                dst_ref=dst,
                send_sem=send_sem,
                recv_sem=recv_sem,
                device_id=(ring(dist),),
                device_id_type=pl.DeviceIdType.MESH,
            )

        def empty(cols, grp):
            return (
                jnp.full((SUB, cols), KEY_MIN, jnp.int32),
                jnp.zeros((SUB, cols), jnp.int32) + grp,
            )

        def scan(load, grp0, g0, n_groups, state):
            unroll = max(u for u in range(1, MAX_UNROLL + 1) if n_groups % u == 0)

            def body(t, carry):
                for u in range(unroll):
                    g = g0 + t * unroll + u
                    cur = jnp.full(carry[1].shape, grp0 + g, jnp.int32)
                    carry = _step(load(g), cur, *carry)
                return carry

            return lax.fori_loop(0, n_groups // unroll, body, state)

        def scan_own(i, state):
            r0, rows, c0, cols = pieces[i]

            def load(g):
                return buf[pl.ds(pl.multiple_of(g * SUB, SUB), SUB), pl.ds(c0, cols)]

            return scan(load, my_grp0, r0 // SUB, rows // SUB, state)

        def scan_own_chains(i, chains):
            r0, rows, c0, cols = pieces[i]
            chains = list(chains)
            for t in range(rows // SUB):
                xg = buf[pl.ds(r0 + t * SUB, SUB), pl.ds(c0, cols)]
                cur = jnp.full((SUB, cols), my_grp0 + r0 // SUB + t, jnp.int32)
                chains[t % len(chains)] = _step(xg, cur, *chains[t % len(chains)])
            return chains

        def scan_peers():
            theirs = []
            for k, dist in enumerate((N_DEV - 1, 1)):
                grp0 = ring(dist) * groups_per_dev + k * (PEER_ROWS // SUB)

                def load(g, k=k):
                    return peer[k, pl.ds(pl.multiple_of(g * SUB, SUB), SUB), :]

                theirs.append(scan(load, grp0, 0, PEER_ROWS // SUB, empty(n, grp0)))
            return _merge(theirs)

        def finish_local(states, dst):
            sub = lax.broadcasted_iota(jnp.int32, (SUB, dst.shape[1]), 0)
            top = jnp.max(_tree(jnp.maximum, [k for k, _ in states]), axis=0, keepdims=True)
            rows = [
                jnp.where(k == top, (grp * SUB + sub).astype(jnp.float32), NO_ROW)
                for k, grp in states
            ]
            idx = jnp.min(_tree(jnp.minimum, rows), axis=0, keepdims=True)
            dst[0:1, :] = top
            dst[1:2, :] = pltpu.bitcast(idx, jnp.int32)
            return top, idx

        def send_partial(src, dst, send_sem, recv_sem):
            copies = [remote(src, dst.at[d - 1], send_sem, recv_sem, d) for d in SEND_ORDER]
            for c in copies:
                c.start()
            return copies

        def finish_global(mine, recv, c0, cols):
            parts = [mine] + [
                (recv[s, 0:1, :], pltpu.bitcast(recv[s, 1:2, :], jnp.float32))
                for s in range(N_DEV - 1)
            ]
            top, idx = _merge(parts)
            o_ref[0:1, pl.ds(c0, cols)] = _unkey(top)
            o_ref[1:2, pl.ds(c0, cols)] = idx

        def run(in_sems, send_sem, peer_sem, recv_a_sem, recv_b_sem):
            def fetch(i):
                r0, rows, c0, cols = pieces[i]
                return pltpu.make_async_copy(
                    x_hbm.at[pl.ds(r0, rows), pl.ds(c0, cols)],
                    buf.at[pl.ds(r0, rows), pl.ds(c0, cols)],
                    in_sems.at[i % N_IN_SEMS],
                )

            for i in range(N_IN_SEMS):
                fetch(i).start()

            barrier = pltpu.get_barrier_semaphore()
            for dist in range(1, N_DEV):
                pl.semaphore_signal(
                    barrier, inc=1, device_id=(ring(dist),), device_id_type=pl.DeviceIdType.MESH
                )
            pl.semaphore_wait(barrier, N_DEV - 1)

            sends = []
            for k, dist in enumerate((1, N_DEV - 1)):
                src = x_hbm.at[pl.ds(k * PEER_ROWS, PEER_ROWS)]
                sends.append(remote(src, peer.at[k], send_sem, peer_sem, dist))
                sends[-1].start()

            state = state_a = chains_b = peer_a = peer_b = mine_a = None
            for i in range(n_pieces):
                fetch(i).wait()
                if i + N_IN_SEMS < n_pieces:
                    fetch(i + N_IN_SEMS).start()
                if i < n_full:
                    if i == 0:
                        state = empty(n, my_grp0 + pieces[0][0] // SUB)
                    state = scan_own(i, state)
                    if i == n_full - 1:
                        state_a = (state[0][:, :cols_a], state[1][:, :cols_a])
                        chains_b = [(state[0][:, cols_a:], state[1][:, cols_a:])]
                        chains_b += [empty(COLS_B, NO_ROW) for _ in range(N_CHAINS - 1)]
                elif i < n_full + n_a:
                    state_a = scan_own(i, state_a)
                else:
                    chains_b = scan_own_chains(i, chains_b)
                    if i == n_pieces - 2:
                        chains_b = [_merge(chains_b)]

                if i == n_full:
                    pltpu.make_async_copy(peer, peer, peer_sem).wait()
                    vmax, grp = scan_peers()
                    peer_a = (vmax[:, :cols_a], grp[:, :cols_a])
                    peer_b = (vmax[:, cols_a:], grp[:, cols_a:])
                if i == n_full + n_a - 1:
                    mine_a = finish_local([state_a, peer_a], send_a)
                    sends += send_partial(send_a, recv_a, send_sem, recv_a_sem)

            mine_b = finish_local([chains_b[0], peer_b], send_b)
            last_sends = send_partial(send_b, recv_b, send_sem, recv_b_sem)

            pltpu.make_async_copy(recv_a, recv_a, recv_a_sem).wait()
            finish_global(mine_a, recv_a, 0, cols_a)
            pltpu.make_async_copy(recv_b, recv_b, recv_b_sem).wait()
            finish_global(mine_b, recv_b, cols_a, COLS_B)
            for c in sends + last_sends:
                c.wait_send()

        pl.run_scoped(
            run,
            pltpu.SemaphoreType.DMA((N_IN_SEMS,)),
            pltpu.SemaphoreType.DMA,
            pltpu.SemaphoreType.DMA,
            pltpu.SemaphoreType.DMA,
            pltpu.SemaphoreType.DMA,
        )

    return pl.pallas_call(
        kernel_body,
        out_shape=jax.ShapeDtypeStruct((2, n), jnp.float32),
        in_specs=[pl.BlockSpec(memory_space=pl.ANY)],
        out_specs=pl.BlockSpec(memory_space=pltpu.VMEM),
        scratch_shapes=[
            pltpu.VMEM((m, n), jnp.float32),
            pltpu.VMEM((2, PEER_ROWS, n), jnp.float32),
            pltpu.VMEM((2, cols_a), jnp.int32),
            pltpu.VMEM((2, COLS_B), jnp.int32),
            pltpu.VMEM((N_DEV - 1, 2, cols_a), jnp.int32),
            pltpu.VMEM((N_DEV - 1, 2, COLS_B), jnp.int32),
        ],
        compiler_params=pltpu.CompilerParams(
            vmem_limit_bytes=64 * 1024 * 1024,
            collective_id=0,
        ),
    )(x)
```
